```python
import numpy as np

kernel_name = "dist_sum_ax1_xy_m512_n256"

def setup_inputs():
    return {"x": np.random.randn(1024, 512).astype(np.float32)}

def reference(x: np.ndarray) -> np.ndarray:
    return np.sum(x, axis=1, keepdims=True)
```

```python
import jax
import jax.numpy as jnp
from jax import lax
from jax.experimental import pallas as pl
from jax.experimental.pallas import tpu as pltpu

_LANES = 128
_SUBLANES = 8
_CHUNKS = (192, 128, 104, 88)
_SENDS = ((0, 3), (3, 4))


def pallas_dist_sum_ax1_xy_m512_n256_kernel(
x: jax.Array,
):
    m, n = x.shape
    assert sum(_CHUNKS) == m and n % _LANES == 0 and _SENDS[-1][1] * _LANES == m
    offs = [sum(_CHUNKS[:i]) for i in range(len(_CHUNKS))]
    n_groups = m // _LANES

    def body(x_hbm, o_ref, xbuf, part, recv, in_sems, send_sems, recv_sems):
        loads = []
        for i, (off, rows) in enumerate(zip(offs, _CHUNKS)):
            cp = pltpu.make_async_copy(
                x_hbm.at[pl.ds(off, rows)], xbuf.at[pl.ds(off, rows)], in_sems.at[i])
            cp.start()
            loads.append(cp)

        peer = (lax.axis_index("x"), 1 - lax.axis_index("y"))
        barrier = pltpu.get_barrier_semaphore()
        pl.semaphore_signal(barrier, inc=1, device_id=peer,
                            device_id_type=pl.DeviceIdType.MESH)

        lane = lax.broadcasted_iota(jnp.int32, (_SUBLANES, _LANES), 1)
        sub = lax.broadcasted_iota(jnp.int32, (_SUBLANES, _LANES), 0)
        lane_blk = lane // _SUBLANES
        diag = (lane % _SUBLANES) == sub

        acc = [None] * n_groups
        sends = []
        done = 0
        for i, (off, rows) in enumerate(zip(offs, _CHUNKS)):
            loads[i].wait()
            for r in range(off, off + rows, _SUBLANES):
                v = xbuf[pl.ds(r, _SUBLANES), pl.ds(0, _LANES)]
                for c in range(_LANES, n, _LANES):
                    v = v + xbuf[pl.ds(r, _SUBLANES), pl.ds(c, _LANES)]
                s = jnp.broadcast_to(jnp.sum(v, axis=1, keepdims=True),
                                     (_SUBLANES, _LANES))
                g, j = r // _LANES, (r % _LANES) // _SUBLANES
                acc[g] = s if acc[g] is None else jnp.where(lane_blk == j, s, acc[g])
            if i == 0:
                pl.semaphore_wait(barrier, 1)
            while (done + 1) * _LANES <= off + rows:
                part[:, pl.ds(done * _LANES, _LANES)] = jnp.sum(
                    jnp.where(diag, acc[done], 0.0), axis=0, keepdims=True)
                done += 1
                for k, (lo, hi) in enumerate(_SENDS):
                    if hi == done:
                        sl = pl.ds(lo * _LANES, (hi - lo) * _LANES)
                        rc = pltpu.make_async_remote_copy(
                            part.at[:, sl], recv.at[:, sl],
                            send_sems.at[k], recv_sems.at[k],
                            device_id=peer, device_id_type=pl.DeviceIdType.MESH)
                        rc.start()
                        sends.append((rc, sl))

        for rc, sl in sends[:-1]:
            rc.wait_recv()
            o_ref[:, sl] = part[:, sl] + recv[:, sl]
        for rc, _ in sends:
            rc.wait_send()
        rc, sl = sends[-1]
        mine = part[:, sl]
        rc.wait_recv()
        o_ref[:, sl] = mine + recv[:, sl]

    out = pl.pallas_call(
        body,
        out_shape=jax.ShapeDtypeStruct((1, m), x.dtype),
        in_specs=[pl.BlockSpec(memory_space=pl.ANY)],
        out_specs=pl.BlockSpec(memory_space=pltpu.VMEM),
        scratch_shapes=[
            pltpu.VMEM((m, n), x.dtype),
            pltpu.VMEM((1, m), x.dtype),
            pltpu.VMEM((1, m), x.dtype),
            pltpu.SemaphoreType.DMA((len(_CHUNKS),)),
            pltpu.SemaphoreType.DMA((len(_SENDS),)),
            pltpu.SemaphoreType.DMA((len(_SENDS),)),
        ],
        compiler_params=pltpu.CompilerParams(
            collective_id=0,
            disable_bounds_checks=True,
            disable_semaphore_checks=True,
        ),
    )(x)
    return out.reshape(m, 1)
```

```python
import jax
import jax.numpy as jnp
from jax import lax
from jax.experimental import pallas as pl
from jax.experimental.pallas import tpu as pltpu

_LANES = 128
_SUBLANES = 8
_STEPS = (
    ((480, 32), (0, 120)),
    ((120, 120),),
    ((240, 96),),
    ((336, 72),),
    ((408, 72),),
)
_SENDS = ((0, 3), (3, 4))


def pallas_dist_sum_ax1_xy_m512_n256_kernel(
x: jax.Array,
):
    m, n = x.shape
    chunks = [c for step in _STEPS for c in step]
    n_groups = m // _LANES
    assert sorted(r for o, k in chunks for r in range(o, o + k)) == list(range(m))
    assert n % _LANES == 0 and _SENDS[-1][1] == n_groups

    def body(x_hbm, o_ref, xbuf, part, recv, in_sems, send_sems, recv_sems):
        loads = []
        for i, (off, rows) in enumerate(chunks):
            cp = pltpu.make_async_copy(
                x_hbm.at[pl.ds(off, rows)], xbuf.at[pl.ds(off, rows)], in_sems.at[i])
            cp.start()
            loads.append(cp)

        peer = (lax.axis_index("x"), 1 - lax.axis_index("y"))
        barrier = pltpu.get_barrier_semaphore()
        pl.semaphore_signal(barrier, inc=1, device_id=peer,
                            device_id_type=pl.DeviceIdType.MESH)

        lane = lax.broadcasted_iota(jnp.int32, (_SUBLANES, _LANES), 1)
        lane_blk = lane >> 3
        lane_bit = [(lane & (1 << b)) != 0 for b in range(3)]

        acc = [None] * n_groups
        filled = [0] * n_groups
        stored = [False] * n_groups
        sends = {}
        next_load = 0
        for step_id, step in enumerate(_STEPS):
            for _ in step:
                loads[next_load].wait()
                next_load += 1
            for off, rows in step:
                for r in range(off, off + rows, _SUBLANES):
                    v = xbuf[pl.ds(r, _SUBLANES), pl.ds(0, _LANES)]
                    for c in range(_LANES, n, _LANES):
                        v = v + xbuf[pl.ds(r, _SUBLANES), pl.ds(c, _LANES)]
                    s = jnp.broadcast_to(
                        jnp.sum(v, axis=1, keepdims=True), (_SUBLANES, _LANES))
                    g, j = divmod(r // _SUBLANES, _LANES // _SUBLANES)
                    acc[g] = s if acc[g] is None else jnp.where(lane_blk == j, s, acc[g])
                    filled[g] += _SUBLANES
            if step_id == 0:
                pl.semaphore_wait(barrier, 1)
            for g in range(n_groups):
                if stored[g] or filled[g] < _LANES:
                    continue
                a = acc[g]
                for b in (2, 1, 0):
                    a = jnp.where(lane_bit[b], pltpu.roll(a, _SUBLANES - (1 << b), 0), a)
                part[:, pl.ds(g * _LANES, _LANES)] = a[0:1, :]
                stored[g] = True
                for k, (lo, hi) in enumerate(_SENDS):
                    if k not in sends and all(stored[lo:hi]):
                        sl = pl.ds(lo * _LANES, (hi - lo) * _LANES)
                        rc = pltpu.make_async_remote_copy(
                            part.at[:, sl], recv.at[:, sl],
                            send_sems.at[k], recv_sems.at[k],
                            device_id=peer, device_id_type=pl.DeviceIdType.MESH)
                        rc.start()
                        sends[k] = (rc, sl)

        *early, (last, last_sl) = sends.values()
        for rc, sl in early:
            rc.wait_recv()
            o_ref[:, sl] = part[:, sl] + recv[:, sl]
        for rc, _ in sends.values():
            rc.wait_send()
        mine = part[:, last_sl]
        last.wait_recv()
        o_ref[:, last_sl] = mine + recv[:, last_sl]

    out = pl.pallas_call(
        body,
        out_shape=jax.ShapeDtypeStruct((1, m), x.dtype),
        in_specs=[pl.BlockSpec(memory_space=pl.ANY)],
        out_specs=pl.BlockSpec(memory_space=pltpu.VMEM),
        scratch_shapes=[
            pltpu.VMEM((m, n), x.dtype),
            pltpu.VMEM((1, m), x.dtype),
            pltpu.VMEM((1, m), x.dtype),
            pltpu.SemaphoreType.DMA((len(chunks),)),
            pltpu.SemaphoreType.DMA((len(_SENDS),)),
            pltpu.SemaphoreType.DMA((len(_SENDS),)),
        ],
        compiler_params=pltpu.CompilerParams(
            collective_id=0,
            disable_semaphore_checks=True,
        ),
    )(x)
    return out.reshape(m, 1)
```

```python
import jax
import jax.numpy as jnp
from jax import lax
from jax.experimental import pallas as pl
from jax.experimental.pallas import tpu as pltpu

_LANES = 128
_SUBLANES = 8
_STEPS = (
    ((480, 32), (0, 120)),
    ((120, 120),),
    ((240, 96),),
    ((336, 72),),
    ((408, 72),),
)
_SENDS = ((0, 3), (3, 4))


def pallas_dist_sum_ax1_xy_m512_n256_kernel(
x: jax.Array,
):
    m, n = x.shape
    chunks = [c for step in _STEPS for c in step]
    n_groups = m // _LANES
    assert sorted(r for o, k in chunks for r in range(o, o + k)) == list(range(m))
    assert n % _LANES == 0 and _SENDS[-1][1] == n_groups

    def body(x_hbm, o_ref, xbuf, part, recv, in_sems, send_sems, recv_sems):
        loads = []
        for i, (off, rows) in enumerate(chunks):
            cp = pltpu.make_async_copy(
                x_hbm.at[pl.ds(off, rows)], xbuf.at[pl.ds(off, rows)], in_sems.at[i])
            cp.start()
            loads.append(cp)

        peer = (lax.axis_index("x"), 1 - lax.axis_index("y"))
        barrier = pltpu.get_barrier_semaphore()
        pl.semaphore_signal(barrier, inc=1, device_id=peer,
                            device_id_type=pl.DeviceIdType.MESH)

        lane_blk = lax.broadcasted_iota(jnp.int32, (_SUBLANES, _LANES), 1) >> 3
        keep_low = {
            h: (lax.broadcasted_iota(jnp.int32, (h, _LANES), 1) & h) == 0
            for h in (4, 2, 1)
        }

        acc = [None] * n_groups
        filled = [0] * n_groups
        stored = [False] * n_groups
        sends = {}
        next_load = 0
        for step_id, step in enumerate(_STEPS):
            for _ in step:
                loads[next_load].wait()
                next_load += 1
            for off, rows in step:
                for r in range(off, off + rows, _SUBLANES):
                    v = xbuf[pl.ds(r, _SUBLANES), pl.ds(0, _LANES)]
                    for c in range(_LANES, n, _LANES):
                        v = v + xbuf[pl.ds(r, _SUBLANES), pl.ds(c, _LANES)]
                    s = jnp.broadcast_to(
                        jnp.sum(v, axis=1, keepdims=True), (_SUBLANES, _LANES))
                    g, j = divmod(r // _SUBLANES, _LANES // _SUBLANES)
                    acc[g] = s if acc[g] is None else jnp.where(lane_blk == j, s, acc[g])
                    filled[g] += _SUBLANES
            if step_id == 0:
                pl.semaphore_wait(barrier, 1)
            for g in range(n_groups):
                if stored[g] or filled[g] < _LANES:
                    continue
                a = acc[g]
                for h in (4, 2, 1):
                    a = jnp.where(keep_low[h], a[:h], a[h:])
                part[:, pl.ds(g * _LANES, _LANES)] = a
                stored[g] = True
                for k, (lo, hi) in enumerate(_SENDS):
                    if k not in sends and all(stored[lo:hi]):
                        sl = pl.ds(lo * _LANES, (hi - lo) * _LANES)
                        rc = pltpu.make_async_remote_copy(
                            part.at[:, sl], recv.at[:, sl],
                            send_sems.at[k], recv_sems.at[k],
                            device_id=peer, device_id_type=pl.DeviceIdType.MESH)
                        rc.start()
                        sends[k] = (rc, sl)

        *early, (last, last_sl) = sends.values()
        for rc, sl in early:
            rc.wait_recv()
            o_ref[:, sl] = part[:, sl] + recv[:, sl]
        for rc, _ in sends.values():
            rc.wait_send()
        mine = part[:, last_sl]
        last.wait_recv()
        o_ref[:, last_sl] = mine + recv[:, last_sl]

    params = dict(collective_id=0)
    if hasattr(pltpu.CompilerParams, "disable_semaphore_checks"):
        params["disable_semaphore_checks"] = True

    out = pl.pallas_call(
        body,
        out_shape=jax.ShapeDtypeStruct((1, m), x.dtype),
        in_specs=[pl.BlockSpec(memory_space=pl.ANY)],
        out_specs=pl.BlockSpec(memory_space=pltpu.VMEM),
        scratch_shapes=[
            pltpu.VMEM((m, n), x.dtype),
            pltpu.VMEM((1, m), x.dtype),
            pltpu.VMEM((1, m), x.dtype),
            pltpu.SemaphoreType.DMA((len(chunks),)),
            pltpu.SemaphoreType.DMA((len(_SENDS),)),
            pltpu.SemaphoreType.DMA((len(_SENDS),)),
        ],
        compiler_params=pltpu.CompilerParams(**params),
    )(x)
    return out.reshape(m, 1)
```

```python
import jax
import jax.numpy as jnp
from jax import lax
from jax.experimental import pallas as pl
from jax.experimental.pallas import tpu as pltpu

_LANES = 128
_SUBLANES = 8
_STEPS = (
    ((480, 32), (0, 120)),
    ((120, 120),),
    ((240, 96),),
    ((336, 72),),
    ((408, 72),),
)
_SENDS = ((0, 3), (3, 4))


def pallas_dist_sum_ax1_xy_m512_n256_kernel(
x: jax.Array,
):
    m, n = x.shape
    chunks = [c for step in _STEPS for c in step]
    n_chunks, n_sends, n_groups = len(chunks), len(_SENDS), m // _LANES
    assert sorted(r for o, k in chunks for r in range(o, o + k)) == list(range(m))
    assert [g for lo, hi in _SENDS for g in range(lo, hi)] == list(range(n_groups))
    assert n % _LANES == 0

    def body(x_hbm, o_ref, *scratch):
        xbufs = scratch[:n_chunks]
        parts = scratch[n_chunks:n_chunks + n_sends]
        recvs = scratch[n_chunks + n_sends:n_chunks + 2 * n_sends]
        in_sems, send_sems, recv_sems = scratch[n_chunks + 2 * n_sends:]

        loads = []
        for i, (off, rows) in enumerate(chunks):
            cp = pltpu.make_async_copy(
                x_hbm.at[pl.ds(off, rows)], xbufs[i], in_sems.at[i])
            cp.start()
            loads.append(cp)

        peer = (lax.axis_index("x"), 1 - lax.axis_index("y"))
        barrier = pltpu.get_barrier_semaphore()
        pl.semaphore_signal(barrier, inc=1, device_id=peer,
                            device_id_type=pl.DeviceIdType.MESH)

        lane_blk = lax.broadcasted_iota(jnp.int32, (_SUBLANES, _LANES), 1) >> 3
        keep_low = {
            h: (lax.broadcasted_iota(jnp.int32, (h, _LANES), 1) & h) == 0
            for h in (4, 2, 1)
        }

        acc = [None] * n_groups
        filled = [0] * n_groups
        stored = [False] * n_groups
        sends = []
        first = 0
        for step_id, step in enumerate(_STEPS):
            for i in range(first, first + len(step)):
                loads[i].wait()
            for i in range(first, first + len(step)):
                off, rows = chunks[i]
                for r in range(0, rows, _SUBLANES):
                    v = xbufs[i][pl.ds(r, _SUBLANES), pl.ds(0, _LANES)]
                    for c in range(_LANES, n, _LANES):
                        v = v + xbufs[i][pl.ds(r, _SUBLANES), pl.ds(c, _LANES)]
                    s = jnp.broadcast_to(
                        jnp.sum(v, axis=1, keepdims=True), (_SUBLANES, _LANES))
                    g, j = divmod((off + r) // _SUBLANES, _LANES // _SUBLANES)
                    acc[g] = s if acc[g] is None else jnp.where(lane_blk == j, s, acc[g])
                    filled[g] += _SUBLANES
            first += len(step)
            if step_id == 0:
                pl.semaphore_wait(barrier, 1)
            for k, (lo, hi) in enumerate(_SENDS):
                for g in range(lo, hi):
                    if stored[g] or filled[g] < _LANES:
                        continue
                    a = acc[g]
                    for h in (4, 2, 1):
                        a = jnp.where(keep_low[h], a[:h], a[h:])
                    parts[k][:, pl.ds((g - lo) * _LANES, _LANES)] = a
                    stored[g] = True
                if k == len(sends) and all(stored[lo:hi]):
                    rc = pltpu.make_async_remote_copy(
                        parts[k], recvs[k], send_sems.at[k], recv_sems.at[k],
                        device_id=peer, device_id_type=pl.DeviceIdType.MESH)
                    rc.start()
                    sends.append(rc)
        assert len(sends) == n_sends

        for k, (lo, hi) in enumerate(_SENDS):
            if k == n_sends - 1:
                for rc in sends:
                    rc.wait_send()
            mine = parts[k][...]
            sends[k].wait_recv()
            o_ref[:, pl.ds(lo * _LANES, (hi - lo) * _LANES)] = mine + recvs[k][...]

    params = dict(collective_id=0)
    if hasattr(pltpu.CompilerParams, "disable_semaphore_checks"):
        params["disable_semaphore_checks"] = True

    sums = [pltpu.VMEM((1, (hi - lo) * _LANES), x.dtype) for lo, hi in _SENDS]
    out = pl.pallas_call(
        body,
        out_shape=jax.ShapeDtypeStruct((1, m), x.dtype),
        in_specs=[pl.BlockSpec(memory_space=pl.ANY)],
        out_specs=pl.BlockSpec(memory_space=pltpu.VMEM),
        scratch_shapes=[pltpu.VMEM((rows, n), x.dtype) for _, rows in chunks]
        + sums
        + sums
        + [
            pltpu.SemaphoreType.DMA((n_chunks,)),
            pltpu.SemaphoreType.DMA((n_sends,)),
            pltpu.SemaphoreType.DMA((n_sends,)),
        ],
        compiler_params=pltpu.CompilerParams(**params),
    )(x)
    return out.reshape(m, 1)
```
